```python
import numpy as np

kernel_name = "dist_mlpseq_tp1d_rep_rep_b128_d128_h256"

def setup_inputs():
    x = np.random.randn(128, 128).astype(np.float32)
    Win0 = np.random.randn(128, 1024).astype(np.float32)
    Wout0 = np.random.randn(1024, 128).astype(np.float32)
    Win1 = np.random.randn(128, 1024).astype(np.float32)
    Wout1 = np.random.randn(1024, 128).astype(np.float32)
    Win2 = np.random.randn(128, 1024).astype(np.float32)
    Wout2 = np.random.randn(1024, 128).astype(np.float32)
    return {"x": x, "Win0": Win0, "Wout0": Wout0, "Win1": Win1, "Wout1": Wout1, "Win2": Win2, "Wout2": Wout2}

def reference(x, Win0, Win1, Win2, Wout0, Wout1, Wout2):
    h = x @ Win0
    h = np.maximum(h, 0.0)
    x = h @ Wout0
    h = x @ Win1
    h = np.maximum(h, 0.0)
    x = h @ Wout1
    h = x @ Win2
    h = np.maximum(h, 0.0)
    x = h @ Wout2
    return x
```

```python
import jax
import jax.numpy as jnp
from jax import lax
from jax.experimental import pallas as pl
from jax.experimental.pallas import tpu as pltpu

MESH = pl.DeviceIdType.MESH
CHUNK = 32
XOR = {"d": 2, "x": 3, "y": 1}
SLOT = {"d": 0, "x": 1, "y": 2}


def _lagged(nc, first, second, late, lag):
    steps = []
    for c in range(nc):
        if lag == 0:
            s = [(first, c), (late, c), (second, c)]
        else:
            s = [(first, c), (second, c)]
            if c - lag >= 0:
                s.append((late, c - lag))
            if c == nc - 1:
                s += [(late, q) for q in range(max(nc - lag, 0), nc)]
        steps.append(s)
    return steps


def pallas_dist_mlpseq_tp1d_rep_rep_b128_d128_h256_kernel(
    x: jax.Array,
    Win0: jax.Array,
    Wout0: jax.Array,
    Win1: jax.Array,
    Wout1: jax.Array,
    Win2: jax.Array,
    Wout2: jax.Array,
):
    B, D = x.shape
    H = Win0.shape[1]
    R = CHUNK
    NC = B // R
    rng = list(range(NC))
    bf16, f32 = jnp.bfloat16, jnp.float32

    sched = {
        1: [_lagged(NC, "d", "y", "x", 1)] * 4,
        2: [
            _lagged(NC, "d", "y", "x", 1),
            _lagged(NC, "y", "x", "d", 0),
            _lagged(NC, "d", "y", "x", NC),
            _lagged(NC, "x", "y", "d", NC),
        ],
    }
    first = {
        0: ("", "W " + " ".join(f"x{c} y{c}" for c in rng) + " V " + " ".join(f"d{c}" for c in rng)),
        1: ("y0", " ".join(f"y{c}" for c in rng[1:]) + " W " + " ".join(f"d{c} x{c}" for c in rng)),
        2: ("d0 y0", " ".join(f"d{c} y{c} x{c - 1}" for c in rng[1:]) + f" x{NC - 1}"),
        3: ("x0", "x1 W " + " ".join(f"d{c} y{c}" + (f" x{c + 2}" if c + 2 < NC else "") for c in rng)),
    }

    def body(x_hbm, wi0, wo0, wi1, wo1, wi2, wo2, out_ref,
             xv, wiv, wov, wib, wob, pbuf, sbuf, rbuf,
             in_sems, send_sems, recv_sems, sem_ab, sem_d):
        me = lax.axis_index("i")
        barrier = pltpu.get_barrier_semaphore()

        def sig(sem, dev):
            pl.semaphore_signal(sem, inc=1, device_id=(dev,), device_id_type=MESH)

        cx0 = pltpu.make_async_copy(x_hbm.at[pl.ds(0, R)], xv.at[pl.ds(0, R)], in_sems.at[0])
        cx1 = pltpu.make_async_copy(x_hbm.at[pl.ds(R, B - R)], xv.at[pl.ds(R, B - R)], in_sems.at[1])
        cw = [
            (pltpu.make_async_copy(wi, wiv.at[l], in_sems.at[2 + 2 * l]),
             pltpu.make_async_copy(wo, wov.at[l], in_sems.at[3 + 2 * l]))
            for l, (wi, wo) in enumerate(((wi0, wo0), (wi1, wo1), (wi2, wo2)))
        ]
        cx0.start()
        cw[0][0].start()
        cw[0][1].start()
        cx1.start()

        @pl.when(me == 0)
        def _():
            sig(barrier, 2)
            sig(barrier, 1)
            sig(barrier, 3)

        @pl.when((me & 1) == 1)
        def _():
            sig(barrier, 2)
            pl.semaphore_wait(barrier, 1)
            sig(sem_ab, 0)

        @pl.when(me == 2)
        def _():
            sig(barrier, 0)
            pl.semaphore_wait(barrier, 3)
            sig(sem_d, 1)
            sig(sem_d, 3)

        def rcopy(l, kind, c):
            return pltpu.make_async_remote_copy(
                src_ref=sbuf.at[l, pl.ds(c * R, R)],
                dst_ref=rbuf.at[l, pl.ds((3 * c + SLOT[kind]) * R, R)],
                send_sem=send_sems.at[l], recv_sem=recv_sems.at[l, c],
                device_id=(me ^ XOR[kind],), device_id_type=MESH)

        def wait_all(buf, sem):
            pltpu.make_async_copy(buf, buf, sem).wait()

        def run_seq(seq, role):
            for tok in seq.split():
                if tok == "W":
                    if role == 0:
                        pl.semaphore_wait(sem_ab, 2)
                    else:
                        pl.semaphore_wait(sem_d, 1)
                elif tok == "V":
                    pl.semaphore_wait(barrier, 1)
                else:
                    rcopy(0, tok[0], int(tok[1:])).start()

        def emit(l, c, p):
            rows = pl.ds(c * R, p.shape[0])
            pbuf[rows, :] = p
            sbuf[l, rows, :] = p.astype(bf16)

        cx0.wait()
        cw[0][0].wait()
        for l in (1, 2):
            cw[l][0].start()
            cw[l][1].start()
        wib[0] = wiv[0].astype(bf16)
        h = jnp.dot(xv[pl.ds(0, R), :].astype(bf16), wib[0], preferred_element_type=f32)
        h = jnp.maximum(h, 0.0).astype(bf16)
        cw[0][1].wait()
        wob[0] = wov[0].astype(bf16)
        emit(0, 0, jnp.dot(h, wob[0], preferred_element_type=f32))
        for r in (2, 1, 3):
            @pl.when(me == r)
            def _():
                run_seq(first[r][0], r)

        cx1.wait()
        h = jnp.dot(xv[pl.ds(R, B - R), :].astype(bf16), wib[0], preferred_element_type=f32)
        h = jnp.maximum(h, 0.0).astype(bf16)
        emit(0, 1, jnp.dot(h, wob[0], preferred_element_type=f32))
        for r in (2, 1, 3, 0):
            @pl.when(me == r)
            def _():
                run_seq(first[r][1], r)

        for l in range(1, 4):
            if l < 3:
                cw[l][0].wait()
                cw[l][1].wait()
                wib[l] = wiv[l].astype(bf16)
                wob[l] = wov[l].astype(bf16)
            if l > 1:
                wait_all(rbuf.at[l - 2], send_sems.at[l - 2])
            for c in range(NC):
                rows = pl.ds(c * R, R)
                wait_all(rbuf.at[l - 1, pl.ds(3 * c * R, 3 * R)], recv_sems.at[l - 1, c])
                s = pbuf[rows, :]
                for j in (2, 1, 0):
                    s = s + rbuf[l - 1, pl.ds((3 * c + j) * R, R), :].astype(f32)
                if l == 3:
                    out_ref[rows, :] = s
                    continue
                h = jnp.dot(s.astype(bf16), wib[l], preferred_element_type=f32)
                h = jnp.maximum(h, 0.0).astype(bf16)
                emit(l, c, jnp.dot(h, wob[l], preferred_element_type=f32))
                orders = [sched[l][r][c] for r in range(4)]
                if all(o == orders[0] for o in orders):
                    for kind, q in orders[0]:
                        rcopy(l, kind, q).start()
                else:
                    for r in range(4):
                        @pl.when(me == r)
                        def _():
                            for kind, q in orders[r]:
                                rcopy(l, kind, q).start()
        wait_all(rbuf.at[2], send_sems.at[2])

    return pl.pallas_call(
        body,
        out_shape=jax.ShapeDtypeStruct((B, D), f32),
        in_specs=[pl.BlockSpec(memory_space=pltpu.HBM)] * 7,
        out_specs=pl.BlockSpec(memory_space=pltpu.VMEM),
        scratch_shapes=[
            pltpu.VMEM((B, D), f32),
            pltpu.VMEM((3, D, H), f32),
            pltpu.VMEM((3, H, D), f32),
            pltpu.VMEM((3, D, H), bf16),
            pltpu.VMEM((3, H, D), bf16),
            pltpu.VMEM((B, D), f32),
            pltpu.VMEM((3, B, D), bf16),
            pltpu.VMEM((3, 3 * B, D), bf16),
            pltpu.SemaphoreType.DMA((8,)),
            pltpu.SemaphoreType.DMA((3,)),
            pltpu.SemaphoreType.DMA((3, NC)),
            pltpu.SemaphoreType.REGULAR,
            pltpu.SemaphoreType.REGULAR,
        ],
        compiler_params=pltpu.CompilerParams(
            collective_id=0,
            disable_bounds_checks=True,
            disable_semaphore_checks=True,
        ),
    )(x, Win0, Wout0, Win1, Wout1, Win2, Wout2)
```

```python
import jax
import jax.numpy as jnp
from jax import lax
from jax.experimental import pallas as pl
from jax.experimental.pallas import tpu as pltpu

MESH = pl.DeviceIdType.MESH
R_, A_, D_, B_ = 0, 1, 2, 3
PEER_XOR = {"d": 2, "x": 3, "y": 1}
SLOTS = {R_: (D_, B_, A_), A_: (B_, D_, R_), B_: (A_, D_, R_), D_: (A_, B_, R_)}
HELLO = {R_: (D_, A_, B_), A_: (B_, D_, R_), B_: (A_, D_, R_), D_: (A_, B_)}
ROWS = 32
N_CHUNKS = 4
N_LONG = 2

LAYER0 = {
    R_: ("", "H x0 y1 x1 x2 a1 x3 a2 y0 b1 a3 b0 a0 b3 b2"),
    A_: ("", "H d0 x0 d1 x1 d2 x3 y1 y0 d3 x2"),
    D_: ("d0 y0", "y3 d1 y1 y2 x0 x2 x1 x3"),
    B_: ("", "H d0 d1 r0 x0 x1 y0 r1 r2 d2 y1 r3 d3 y2 y3"),
}
LAYER1 = {
    R_: (((0,), "d0 y0"), ((1,), "d1 y1 x1 x0")),
    A_: (((0,), "d0 x0"), ((1,), "x1 y0 d1"), ((2,), "d2 y2 x2"), ((3,), "x3 y1 y3 d3")),
    D_: (((0,), "y0 d0"), ((1,), "x0 y1 d1"), ((2, 3), "x1 x2 y3 d3 d2 y2 x3")),
    B_: (((0,), "d0 y0"), ((1,), "d1 y1"), ((2,), "d2"), ((3,), "d3 x0 x1 y3 x2 x3 y2")),
}
LAYER2 = {
    R_: (((0, 1), "d1 d0 y1"), ((2, 3), "y2 x1 x2 y3 x0 x3 d2 y0 d3")),
    A_: (((0,), "y0"), ((1,), "y1"), ((2,), "d0 x0 y2"), ((3,), "d2 y3 d1 x1 d3 x2 x3")),
    D_: (((0,), "d0"), ((1,), "d1"), ((2, 3), "y1 d2 d3 x3 y0 x2 x0 y2 x1 y3")),
    B_: (((0,), "d0 x0"), ((1, 2), "x1 x2"), ((3,), "y0 y1 x3 y2 y3 d2 d1 d3")),
}


def _senders(layer, dst, c):
    if layer == 0:
        direct_from_r = dst == A_ and c < N_LONG
        return [s for s in SLOTS[dst] if s != R_ or direct_from_r]
    if layer == 1:
        return [s for s in SLOTS[dst] if s != R_ or c < N_LONG]
    return list(SLOTS[dst])


def pallas_dist_mlpseq_tp1d_rep_rep_b128_d128_h256_kernel(
    x: jax.Array,
    Win0: jax.Array,
    Wout0: jax.Array,
    Win1: jax.Array,
    Wout1: jax.Array,
    Win2: jax.Array,
    Wout2: jax.Array,
):
    B, D = x.shape
    H = Win0.shape[1]
    R = ROWS
    HH = H // 2
    assert B == N_CHUNKS * R and HH == D
    bf16, f32 = jnp.bfloat16, jnp.float32

    def dot(a, b):
        return jnp.dot(a, b, preferred_element_type=f32)

    def body(x_hbm, wi0, wo0, wi1, wo1, wi2, wo2, out_ref,
             xv, wiv, wov, wib, wob, wext, pbuf, sbuf, relay, rbuf,
             in_sems, send_sems, recv_sems, relay_sems, w_send, w_recv, d_ready):
        me = lax.axis_index("i")
        barrier = pltpu.get_barrier_semaphore()

        load_x0 = pltpu.make_async_copy(x_hbm.at[pl.ds(0, R)], xv.at[pl.ds(0, R)], in_sems.at[0])
        load_x1 = pltpu.make_async_copy(x_hbm.at[pl.ds(R, B - R)], xv.at[pl.ds(R, B - R)], in_sems.at[1])
        load_w = [
            (pltpu.make_async_copy(wi, wiv.at[l], in_sems.at[2 + 2 * l]),
             pltpu.make_async_copy(wo, wov.at[l], in_sems.at[3 + 2 * l]))
            for l, (wi, wo) in enumerate(((wi0, wo0), (wi1, wo1), (wi2, wo2)))
        ]
        load_x0.start()
        load_w[0][0].start()
        load_w[0][1].start()
        load_x1.start()

        def signal(sem, dev):
            pl.semaphore_signal(sem, inc=1, device_id=(dev,), device_id_type=MESH)

        def wait_bytes(buf, sem):
            pltpu.make_async_copy(buf, buf, sem).wait()

        def cast_weights(l):
            load_w[l][0].wait()
            load_w[l][1].wait()
            for h in range(2):
                wib[l, h] = wiv[l, :, pl.ds(h * HH, HH)].astype(bf16)
            wob[l] = wov[l].astype(bf16)

        def weights(l):
            return (wib[l, 0], wib[l, 1], wob[l, pl.ds(0, HH), :], wob[l, pl.ds(HH, HH), :])

        def mlp(a, w, extended=False):
            h0 = jnp.maximum(dot(a, w[0]), 0.0).astype(bf16)
            h1 = jnp.maximum(dot(a, w[1]), 0.0).astype(bf16)
            if extended:
                h2 = jnp.maximum(dot(a, wext[0]), 0.0).astype(bf16)
            p = dot(h0, w[2]) + dot(h1, w[3])
            if extended:
                p = p + dot(h2, wext[1])
            return p

        def store_partial(l, row0, p):
            rows = pl.ds(row0, p.shape[0])
            pbuf[rows, :] = p
            sbuf[l, rows, :] = p.astype(bf16)

        def program(me_):
            n_sent = [0, 0, 0]
            done = {"d_ready": False}

            def send_partial(l, kind, c):
                dst = me_ ^ PEER_XOR[kind]
                to_relay = l == 0 and me_ == R_ and dst == B_
                folded = l == 0 and me_ == B_ and (kind == "y" or (kind == "d" and c >= N_LONG))
                rows = pl.ds(c * R, R)
                if me_ == R_ and dst == D_ and not done["d_ready"]:
                    pl.semaphore_wait(d_ready, 1)
                    done["d_ready"] = True
                pltpu.make_async_remote_copy(
                    src_ref=relay.at[rows] if folded else sbuf.at[l, rows],
                    dst_ref=rbuf.at[l, pl.ds((3 * c + SLOTS[dst].index(me_)) * R, R)],
                    send_sem=send_sems.at[l],
                    recv_sem=relay_sems.at[c] if to_relay else recv_sems.at[l, c],
                    device_id=(dst,), device_id_type=MESH,
                ).start()
                n_sent[l] += 1

            def send_weights(dest, piece):
                half = 0 if dest == "a" else 1
                n = D // 2
                if piece < 2:
                    src = wib.at[1, half, pl.ds(piece * n, n)]
                    dst = wext.at[0, pl.ds(piece * n, n)]
                else:
                    src = wob.at[1, pl.ds(half * HH + (piece - 2) * n, n)]
                    dst = wext.at[1, pl.ds((piece - 2) * n, n)]
                pltpu.make_async_remote_copy(
                    src_ref=src, dst_ref=dst, send_sem=w_send, recv_sem=w_recv,
                    device_id=(A_ if dest == "a" else B_,), device_id_type=MESH,
                ).start()

            def run(l, script):
                for tok in script.split():
                    if tok == "H":
                        pl.semaphore_wait(barrier, 2 if me_ == R_ else 3)
                        continue
                    op, i = tok[0], int(tok[1:])
                    if op in "ab":
                        send_weights(op, i)
                    elif op == "r":
                        slot = pl.ds((3 * i + 2) * R, R)
                        wait_bytes(rbuf.at[0, slot], relay_sems.at[i])
                        rows = pl.ds(i * R, R)
                        relay[rows, :] = (pbuf[rows, :] + rbuf[0, slot, :].astype(f32)).astype(bf16)
                    else:
                        send_partial(l, op, i)

            def wait_chunk(l, c):
                n = len(_senders(l, me_, c))
                wait_bytes(rbuf.at[l, pl.ds(3 * c * R, n * R)], recv_sems.at[l, c])

            def reduce_chunk(l, c):
                slots = list(range(len(_senders(l, me_, c))))
                if l == 0 and me_ == B_:
                    slots.append(2)
                own = not (l == 1 and me_ == R_ and c >= N_LONG)
                s = pbuf[pl.ds(c * R, R), :] if own else None
                for j in reversed(slots):
                    v = rbuf[l, pl.ds((3 * c + j) * R, R), :].astype(f32)
                    s = v if s is None else s + v
                return s

            def layer(l, steps):
                have_ext = False
                for chunks, script in steps:
                    w = weights(l)
                    for c in chunks:
                        wait_chunk(l - 1, c)
                    extended = l == 1 and me_ in (A_, B_) and chunks[0] >= N_LONG
                    if extended and not have_ext:
                        wait_bytes(wext, w_recv)
                        have_ext = True
                    a = jnp.concatenate([reduce_chunk(l - 1, c) for c in chunks], axis=0)
                    p = mlp(a.astype(bf16), w, extended)
                    for k, c in enumerate(chunks):
                        store_partial(l, c * R, p[k * R:(k + 1) * R])
                    run(l, script)

            def wait_sends(l):
                wait_bytes(rbuf.at[l, pl.ds(0, n_sent[l] * R)], send_sems.at[l])

            for peer in HELLO[me_]:
                signal(barrier, peer)
            if me_ == D_:
                pl.semaphore_wait(barrier, 3)
                signal(d_ready, R_)

            load_x0.wait()
            load_w[0][0].wait()
            for l in (1, 2):
                load_w[l][0].start()
                load_w[l][1].start()
            for h in range(2):
                wib[0, h] = wiv[0, :, pl.ds(h * HH, HH)].astype(bf16)
            a = xv[pl.ds(0, R), :].astype(bf16)
            h0 = jnp.maximum(dot(a, wib[0, 0]), 0.0).astype(bf16)
            h1 = jnp.maximum(dot(a, wib[0, 1]), 0.0).astype(bf16)
            load_w[0][1].wait()
            w2 = wov[0, pl.ds(0, HH), :].astype(bf16)
            w3 = wov[0, pl.ds(HH, HH), :].astype(bf16)
            wob[0, pl.ds(0, HH), :] = w2
            wob[0, pl.ds(HH, HH), :] = w3
            store_partial(0, 0, dot(h0, w2) + dot(h1, w3))
            run(0, LAYER0[me_][0])
            load_x1.wait()
            store_partial(0, R, mlp(xv[pl.ds(R, B - R), :].astype(bf16), weights(0)))
            if me_ == R_:
                cast_weights(1)
            run(0, LAYER0[me_][1])
            if me_ != R_:
                cast_weights(1)

            layer(1, LAYER1[me_])
            cast_weights(2)
            wait_sends(0)
            if me_ == R_:
                wait_bytes(wib.at[pl.ds(1, 2)], w_send)
            layer(2, LAYER2[me_])
            wait_sends(1)
            for chunks, _ in LAYER2[me_]:
                for c in chunks:
                    wait_chunk(2, c)
                    out_ref[pl.ds(c * R, R), :] = reduce_chunk(2, c)
            wait_sends(2)

        for pos in (D_, A_, B_, R_):
            @pl.when(me == pos)
            def _():
                program(pos)

    return pl.pallas_call(
        body,
        out_shape=jax.ShapeDtypeStruct((B, D), f32),
        in_specs=[pl.BlockSpec(memory_space=pltpu.HBM)] * 7,
        out_specs=pl.BlockSpec(memory_space=pltpu.VMEM),
        scratch_shapes=[
            pltpu.VMEM((B, D), f32),
            pltpu.VMEM((3, D, H), f32),
            pltpu.VMEM((3, H, D), f32),
            pltpu.VMEM((3, 2, D, HH), bf16),
            pltpu.VMEM((3, H, D), bf16),
            pltpu.VMEM((2, D, HH), bf16),
            pltpu.VMEM((B, D), f32),
            pltpu.VMEM((3, B, D), bf16),
            pltpu.VMEM((B, D), bf16),
            pltpu.VMEM((3, 3 * B, D), bf16),
            pltpu.SemaphoreType.DMA((8,)),
            pltpu.SemaphoreType.DMA((3,)),
            pltpu.SemaphoreType.DMA((3, N_CHUNKS)),
            pltpu.SemaphoreType.DMA((N_CHUNKS,)),
            pltpu.SemaphoreType.DMA,
            pltpu.SemaphoreType.DMA,
            pltpu.SemaphoreType.REGULAR,
        ],
        compiler_params=pltpu.CompilerParams(
            collective_id=0,
            disable_bounds_checks=True,
            disable_semaphore_checks=True,
        ),
    )(x, Win0, Wout0, Win1, Wout1, Win2, Wout2)
```

```python
import jax
import jax.numpy as jnp
from jax import lax
from jax.experimental import pallas as pl
from jax.experimental.pallas import tpu as pltpu

MESH = pl.DeviceIdType.MESH
R_, A_, D_, B_ = 0, 1, 2, 3
PEER_XOR = {"d": 2, "x": 3, "y": 1}
SLOTS = {R_: (D_, B_, A_), A_: (B_, D_, R_), B_: (A_, D_, R_), D_: (A_, B_, R_)}
HELLO = {R_: (D_, A_, B_), A_: (B_, D_, R_), B_: (A_, D_, R_), D_: (A_, B_)}
ROWS = 32
N_CHUNKS = 4
N_LONG = 2

LAYER0 = {
    R_: ("", "H x0 y1 x1 x2 a1 x3 a2 y0 b1 a3 b0 a0 b3 b2"),
    A_: ("", "H d0 x0 d1 x1 d2 x3 y1 y0 d3 x2"),
    D_: ("d0 y0", "y3 d1 y1 y2 x0 x2 x1 x3"),
    B_: ("", "H d0 d1 r0 x0 x1 y0 r1 r2 d2 y1 r3 d3 y2 y3"),
}
LAYER1 = {
    R_: (((0,), "d0 y0"), ((1,), "d1 y1 x1 x0")),
    A_: (((0,), "d0 x0"), ((1,), "x1 y0 d1"), ((2,), "d2 y2 x2"), ((3,), "x3 y1 y3 d3")),
    D_: (((0,), "y0 d0"), ((1,), "x0 y1 d1"), ((2, 3), "x1 x2 y3 d3 d2 y2 x3")),
    B_: (((0,), "d0 y0"), ((1,), "d1 y1"), ((2,), "d2"), ((3,), "d3 x0 x1 y3 x2 x3 y2")),
}
LAYER2 = {
    R_: (((0, 1), "d1 d0 y1"), ((2, 3), "y2 x1 x2 y3 x0 x3 d2 y0 d3")),
    A_: (((0,), "y0"), ((1,), "y1"), ((2,), "d0 x0 y2"), ((3,), "d2 y3 d1 x1 d3 x2 x3")),
    D_: (((0,), "d0"), ((1,), "d1"), ((2, 3), "y1 d2 d3 x3 y0 x2 x0 y2 x1 y3")),
    B_: (((0,), "d0 x0"), ((1, 2), "x1 x2"), ((3,), "y0 y1 x3 y2 y3 d2 d1 d3")),
}


def _senders(layer, dst, c):
    if layer == 0:
        direct_from_r = dst == A_ and c < N_LONG
        return [s for s in SLOTS[dst] if s != R_ or direct_from_r]
    if layer == 1:
        return [s for s in SLOTS[dst] if s != R_ or c < N_LONG]
    return list(SLOTS[dst])


def pallas_dist_mlpseq_tp1d_rep_rep_b128_d128_h256_kernel(
    x: jax.Array,
    Win0: jax.Array,
    Wout0: jax.Array,
    Win1: jax.Array,
    Wout1: jax.Array,
    Win2: jax.Array,
    Wout2: jax.Array,
):
    B, D = x.shape
    H = Win0.shape[1]
    R = ROWS
    HH = H // 2
    assert B == N_CHUNKS * R and HH == D
    bf16, f32 = jnp.bfloat16, jnp.float32

    def dot(a, b):
        return jnp.dot(a, b, preferred_element_type=f32)

    def body(x_hbm, wi0, wo0, wi1, wo1, wi2, wo2, out_ref,
             xv, wiv, wov, wib, wob, wext, pbuf, sbuf, relay, rbuf,
             in_sems, send_sems, recv_sems, relay_sems, w_recv, d_ready):
        me = lax.axis_index("i")
        barrier = pltpu.get_barrier_semaphore()

        load_x0 = pltpu.make_async_copy(x_hbm.at[pl.ds(0, R)], xv.at[pl.ds(0, R)], in_sems.at[0])
        load_x1 = pltpu.make_async_copy(x_hbm.at[pl.ds(R, B - R)], xv.at[pl.ds(R, B - R)], in_sems.at[1])
        load_w = [
            (pltpu.make_async_copy(wi, wiv.at[l], in_sems.at[2 + 2 * l]),
             pltpu.make_async_copy(wo, wov.at[l], in_sems.at[3 + 2 * l]))
            for l, (wi, wo) in enumerate(((wi0, wo0), (wi1, wo1), (wi2, wo2)))
        ]
        load_x0.start()
        load_w[0][0].start()
        load_w[0][1].start()
        load_x1.start()

        def signal(sem, dev):
            pl.semaphore_signal(sem, inc=1, device_id=(dev,), device_id_type=MESH)

        def wait_bytes(buf, sem):
            pltpu.make_async_copy(buf, buf, sem).wait()

        def cast_weights(l):
            load_w[l][0].wait()
            load_w[l][1].wait()
            for h in range(2):
                wib[l, h] = wiv[l, :, pl.ds(h * HH, HH)].astype(bf16)
            wob[l] = wov[l].astype(bf16)

        def weights(l):
            return (wib[l, 0], wib[l, 1], wob[l, pl.ds(0, HH), :], wob[l, pl.ds(HH, HH), :])

        def mlp(a, w, extended=False):
            h0 = jnp.maximum(dot(a, w[0]), 0.0).astype(bf16)
            h1 = jnp.maximum(dot(a, w[1]), 0.0).astype(bf16)
            if extended:
                h2 = jnp.maximum(dot(a, wext[0]), 0.0).astype(bf16)
            p = dot(h0, w[2]) + dot(h1, w[3])
            if extended:
                p = p + dot(h2, wext[1])
            return p

        def store_partial(l, row0, p):
            rows = pl.ds(row0, p.shape[0])
            pbuf[rows, :] = p
            sbuf[l, rows, :] = p.astype(bf16)

        def program(me_):
            in_flight = [[], [], []]
            done = {"d_ready": False}

            def send_partial(l, kind, c):
                dst = me_ ^ PEER_XOR[kind]
                to_relay = l == 0 and me_ == R_ and dst == B_
                folded = l == 0 and me_ == B_ and (kind == "y" or (kind == "d" and c >= N_LONG))
                rows = pl.ds(c * R, R)
                if me_ == R_ and dst == D_ and not done["d_ready"]:
                    pl.semaphore_wait(d_ready, 1)
                    done["d_ready"] = True
                copy = pltpu.make_async_remote_copy(
                    src_ref=relay.at[rows] if folded else sbuf.at[l, rows],
                    dst_ref=rbuf.at[l, pl.ds((3 * c + SLOTS[dst].index(me_)) * R, R)],
                    send_sem=send_sems.at[l],
                    recv_sem=relay_sems.at[c] if to_relay else recv_sems.at[l, c],
                    device_id=(dst,), device_id_type=MESH,
                )
                copy.start()
                in_flight[l].append(copy)

            def send_weights(dest, piece):
                half = 0 if dest == "a" else 1
                n = D // 2
                if piece < 2:
                    src = wib.at[1, half, pl.ds(piece * n, n)]
                    dst = wext.at[0, pl.ds(piece * n, n)]
                else:
                    src = wob.at[1, pl.ds(half * HH + (piece - 2) * n, n)]
                    dst = wext.at[1, pl.ds((piece - 2) * n, n)]
                copy = pltpu.make_async_remote_copy(
                    src_ref=src, dst_ref=dst, send_sem=send_sems.at[0], recv_sem=w_recv,
                    device_id=(A_ if dest == "a" else B_,), device_id_type=MESH,
                )
                copy.start()
                in_flight[0].append(copy)

            def run(l, script):
                for tok in script.split():
                    if tok == "H":
                        pl.semaphore_wait(barrier, 2 if me_ == R_ else 3)
                        continue
                    op, i = tok[0], int(tok[1:])
                    if op in "ab":
                        send_weights(op, i)
                    elif op == "r":
                        slot = pl.ds((3 * i + 2) * R, R)
                        wait_bytes(rbuf.at[0, slot], relay_sems.at[i])
                        rows = pl.ds(i * R, R)
                        relay[rows, :] = (pbuf[rows, :] + rbuf[0, slot, :].astype(f32)).astype(bf16)
                    else:
                        send_partial(l, op, i)

            def wait_chunk(l, c):
                n = len(_senders(l, me_, c))
                wait_bytes(rbuf.at[l, pl.ds(3 * c * R, n * R)], recv_sems.at[l, c])

            def reduce_chunk(l, c):
                slots = list(range(len(_senders(l, me_, c))))
                if l == 0 and me_ == B_:
                    slots.append(2)
                own = not (l == 1 and me_ == R_ and c >= N_LONG)
                s = pbuf[pl.ds(c * R, R), :] if own else None
                for j in reversed(slots):
                    v = rbuf[l, pl.ds((3 * c + j) * R, R), :].astype(f32)
                    s = v if s is None else s + v
                return s

            def layer(l, steps):
                have_ext = False
                for chunks, script in steps:
                    w = weights(l)
                    for c in chunks:
                        wait_chunk(l - 1, c)
                    extended = l == 1 and me_ in (A_, B_) and chunks[0] >= N_LONG
                    if extended and not have_ext:
                        wait_bytes(wext, w_recv)
                        have_ext = True
                    a = jnp.concatenate([reduce_chunk(l - 1, c) for c in chunks], axis=0)
                    p = mlp(a.astype(bf16), w, extended)
                    for k, c in enumerate(chunks):
                        store_partial(l, c * R, p[k * R:(k + 1) * R])
                    run(l, script)

            def wait_sends(l):
                for copy in in_flight[l]:
                    copy.wait_send()

            for peer in HELLO[me_]:
                signal(barrier, peer)
            if me_ == D_:
                pl.semaphore_wait(barrier, 3)
                signal(d_ready, R_)

            load_x0.wait()
            load_w[0][0].wait()
            for l in (1, 2):
                load_w[l][0].start()
                load_w[l][1].start()
            for h in range(2):
                wib[0, h] = wiv[0, :, pl.ds(h * HH, HH)].astype(bf16)
            a = xv[pl.ds(0, R), :].astype(bf16)
            h0 = jnp.maximum(dot(a, wib[0, 0]), 0.0).astype(bf16)
            h1 = jnp.maximum(dot(a, wib[0, 1]), 0.0).astype(bf16)
            load_w[0][1].wait()
            w2 = wov[0, pl.ds(0, HH), :].astype(bf16)
            w3 = wov[0, pl.ds(HH, HH), :].astype(bf16)
            wob[0, pl.ds(0, HH), :] = w2
            wob[0, pl.ds(HH, HH), :] = w3
            store_partial(0, 0, dot(h0, w2) + dot(h1, w3))
            run(0, LAYER0[me_][0])
            load_x1.wait()
            store_partial(0, R, mlp(xv[pl.ds(R, B - R), :].astype(bf16), weights(0)))
            if me_ == R_:
                cast_weights(1)
            run(0, LAYER0[me_][1])
            if me_ != R_:
                cast_weights(1)

            layer(1, LAYER1[me_])
            cast_weights(2)
            wait_sends(0)
            layer(2, LAYER2[me_])
            wait_sends(1)
            order = [c for chunks, _ in LAYER2[me_] for c in chunks]
            for c in order:
                if c == order[-1]:
                    wait_sends(2)
                wait_chunk(2, c)
                out_ref[pl.ds(c * R, R), :] = reduce_chunk(2, c)

        for pos in (D_, A_, B_, R_):
            @pl.when(me == pos)
            def _():
                program(pos)

    return pl.pallas_call(
        body,
        out_shape=jax.ShapeDtypeStruct((B, D), f32),
        in_specs=[pl.BlockSpec(memory_space=pltpu.HBM)] * 7,
        out_specs=pl.BlockSpec(memory_space=pltpu.VMEM),
        scratch_shapes=[
            pltpu.VMEM((B, D), f32),
            pltpu.VMEM((3, D, H), f32),
            pltpu.VMEM((3, H, D), f32),
            pltpu.VMEM((3, 2, D, HH), bf16),
            pltpu.VMEM((3, H, D), bf16),
            pltpu.VMEM((2, D, HH), bf16),
            pltpu.VMEM((B, D), f32),
            pltpu.VMEM((3, B, D), bf16),
            pltpu.VMEM((B, D), bf16),
            pltpu.VMEM((3, 3 * B, D), bf16),
            pltpu.SemaphoreType.DMA((8,)),
            pltpu.SemaphoreType.DMA((3,)),
            pltpu.SemaphoreType.DMA((3, N_CHUNKS)),
            pltpu.SemaphoreType.DMA((N_CHUNKS,)),
            pltpu.SemaphoreType.DMA,
            pltpu.SemaphoreType.REGULAR,
        ],
        compiler_params=pltpu.CompilerParams(
            collective_id=0,
            disable_bounds_checks=True,
            disable_semaphore_checks=True,
        ),
    )(x, Win0, Wout0, Win1, Wout1, Win2, Wout2)
```

```python
import dataclasses

import jax
import jax.numpy as jnp
from jax import lax
from jax.experimental import pallas as pl
from jax.experimental.pallas import tpu as pltpu

_SEM = pl if hasattr(pl, "semaphore_signal") else pltpu
MESH = _SEM.DeviceIdType.MESH
R_, A_, D_, B_ = 0, 1, 2, 3
PEER_XOR = {"d": 2, "x": 3, "y": 1}
SLOTS = {R_: (D_, B_, A_), A_: (B_, D_, R_), B_: (A_, D_, R_), D_: (A_, B_, R_)}
HELLO = {R_: (D_, A_, B_), A_: (B_, D_, R_), B_: (A_, D_, R_), D_: (A_, B_)}
ROWS = 32
N_CHUNKS = 4
N_LONG = 2

LAYER0 = {
    R_: ("", "H x0 y1 x1 x2 a1 x3 a2 y0 b1 a3 b0 a0 b3 b2"),
    A_: ("", "H d0 x0 d1 x1 d2 x3 y1 y0 d3 x2"),
    D_: ("d0 y0", "y3 d1 y1 y2 x0 x2 x1 x3"),
    B_: ("", "H d0 d1 r0 x0 x1 y0 r1 r2 d2 y1 r3 d3 y2 y3"),
}
LAYER1 = {
    R_: (((0,), "d0 y0"), ((1,), "d1 y1 x1 x0")),
    A_: (((0,), "d0 x0"), ((1,), "x1 y0 d1"), ((2,), "d2 y2 x2"), ((3,), "x3 y1 y3 d3")),
    D_: (((0,), "y0 d0"), ((1,), "x0 y1 d1"), ((2, 3), "x1 x2 y3 d3 d2 y2 x3")),
    B_: (((0,), "d0 y0"), ((1,), "d1 y1"), ((2,), "d2"), ((3,), "d3 x0 x1 y3 x2 x3 y2")),
}
LAYER2 = {
    R_: (((0, 1), "d1 d0 y1"), ((2, 3), "y2 x1 x2 y3 x0 x3 d2 y0 d3")),
    A_: (((0,), "y0"), ((1,), "y1"), ((2,), "d0 x0 y2"), ((3,), "d2 y3 d1 x1 d3 x2 x3")),
    D_: (((0,), "d0"), ((1,), "d1"), ((2, 3), "y1 d2 d3 x3 y0 x2 x0 y2 x1 y3")),
    B_: (((0,), "d0 x0"), ((1, 2), "x1 x2"), ((3,), "y0 y1 x3 y2 y3 d2 d1 d3")),
}


def _senders(layer, dst, c):
    if layer == 0:
        direct_from_r = dst == A_ and c < N_LONG
        return [s for s in SLOTS[dst] if s != R_ or direct_from_r]
    if layer == 1:
        return [s for s in SLOTS[dst] if s != R_ or c < N_LONG]
    return list(SLOTS[dst])


def pallas_dist_mlpseq_tp1d_rep_rep_b128_d128_h256_kernel(
    x: jax.Array,
    Win0: jax.Array,
    Wout0: jax.Array,
    Win1: jax.Array,
    Wout1: jax.Array,
    Win2: jax.Array,
    Wout2: jax.Array,
):
    B, D = x.shape
    H = Win0.shape[1]
    R = ROWS
    HH = H // 2
    assert B == N_CHUNKS * R and HH == D
    bf16, f32 = jnp.bfloat16, jnp.float32

    def dot(a, b):
        return jnp.dot(a, b, preferred_element_type=f32)

    def body(x_hbm, wi0, wo0, wi1, wo1, wi2, wo2, out_ref,
             xv, wiv, wov, wib, wob, wext, pbuf, sbuf, relay, rbuf,
             in_sems, send_sems, recv_sems, relay_sems, w_recv, d_ready):
        me = lax.axis_index("i")
        barrier = pltpu.get_barrier_semaphore()

        load_x0 = pltpu.make_async_copy(x_hbm.at[pl.ds(0, R)], xv.at[pl.ds(0, R)], in_sems.at[0])
        load_x1 = pltpu.make_async_copy(x_hbm.at[pl.ds(R, B - R)], xv.at[pl.ds(R, B - R)], in_sems.at[1])
        load_w = [
            (pltpu.make_async_copy(wi, wiv.at[l], in_sems.at[2 + 2 * l]),
             pltpu.make_async_copy(wo, wov.at[l], in_sems.at[3 + 2 * l]))
            for l, (wi, wo) in enumerate(((wi0, wo0), (wi1, wo1), (wi2, wo2)))
        ]
        load_x0.start()
        load_w[0][0].start()
        load_w[0][1].start()
        load_x1.start()

        def signal(sem, dev):
            _SEM.semaphore_signal(sem, inc=1, device_id=(dev,), device_id_type=MESH)

        def wait_bytes(buf, sem):
            pltpu.make_async_copy(buf, buf, sem).wait()

        def cast_weights(l):
            load_w[l][0].wait()
            load_w[l][1].wait()
            for h in range(2):
                wib[l, h] = wiv[l, :, pl.ds(h * HH, HH)].astype(bf16)
            wob[l] = wov[l].astype(bf16)

        def weights(l):
            return (wib[l, 0], wib[l, 1], wob[l, pl.ds(0, HH), :], wob[l, pl.ds(HH, HH), :])

        def mlp(a, w, extended=False):
            h0 = jnp.maximum(dot(a, w[0]), 0.0).astype(bf16)
            h1 = jnp.maximum(dot(a, w[1]), 0.0).astype(bf16)
            if extended:
                h2 = jnp.maximum(dot(a, wext[0]), 0.0).astype(bf16)
            p = dot(h0, w[2]) + dot(h1, w[3])
            if extended:
                p = p + dot(h2, wext[1])
            return p

        def store_partial(l, row0, p):
            rows = pl.ds(row0, p.shape[0])
            pbuf[rows, :] = p
            sbuf[l, rows, :] = p.astype(bf16)

        def program(me_):
            in_flight = [[], [], []]
            done = {"d_ready": False}

            def send_partial(l, kind, c):
                dst = me_ ^ PEER_XOR[kind]
                to_relay = l == 0 and me_ == R_ and dst == B_
                folded = l == 0 and me_ == B_ and (kind == "y" or (kind == "d" and c >= N_LONG))
                rows = pl.ds(c * R, R)
                if me_ == R_ and dst == D_ and not done["d_ready"]:
                    _SEM.semaphore_wait(d_ready, 1)
                    done["d_ready"] = True
                copy = pltpu.make_async_remote_copy(
                    src_ref=relay.at[rows] if folded else sbuf.at[l, rows],
                    dst_ref=rbuf.at[l, pl.ds((3 * c + SLOTS[dst].index(me_)) * R, R)],
                    send_sem=send_sems.at[l],
                    recv_sem=relay_sems.at[c] if to_relay else recv_sems.at[l, c],
                    device_id=(dst,), device_id_type=MESH,
                )
                copy.start()
                in_flight[l].append(copy)

            def send_weights(dest, piece):
                half = 0 if dest == "a" else 1
                n = D // 2
                if piece < 2:
                    src = wib.at[1, half, pl.ds(piece * n, n)]
                    dst = wext.at[0, pl.ds(piece * n, n)]
                else:
                    src = wob.at[1, pl.ds(half * HH + (piece - 2) * n, n)]
                    dst = wext.at[1, pl.ds((piece - 2) * n, n)]
                copy = pltpu.make_async_remote_copy(
                    src_ref=src, dst_ref=dst, send_sem=send_sems.at[0], recv_sem=w_recv,
                    device_id=(A_ if dest == "a" else B_,), device_id_type=MESH,
                )
                copy.start()
                in_flight[0].append(copy)

            def run(l, script):
                for tok in script.split():
                    if tok == "H":
                        _SEM.semaphore_wait(barrier, 2 if me_ == R_ else 3)
                        continue
                    op, i = tok[0], int(tok[1:])
                    if op in "ab":
                        send_weights(op, i)
                    elif op == "r":
                        slot = pl.ds((3 * i + 2) * R, R)
                        wait_bytes(rbuf.at[0, slot], relay_sems.at[i])
                        rows = pl.ds(i * R, R)
                        relay[rows, :] = (pbuf[rows, :] + rbuf[0, slot, :].astype(f32)).astype(bf16)
                    else:
                        send_partial(l, op, i)

            def wait_chunk(l, c):
                n = len(_senders(l, me_, c))
                wait_bytes(rbuf.at[l, pl.ds(3 * c * R, n * R)], recv_sems.at[l, c])

            def reduce_chunk(l, c):
                slots = list(range(len(_senders(l, me_, c))))
                if l == 0 and me_ == B_:
                    slots.append(2)
                own = not (l == 1 and me_ == R_ and c >= N_LONG)
                s = pbuf[pl.ds(c * R, R), :] if own else None
                for j in reversed(slots):
                    v = rbuf[l, pl.ds((3 * c + j) * R, R), :].astype(f32)
                    s = v if s is None else s + v
                return s

            def layer(l, steps):
                have_ext = False
                for chunks, script in steps:
                    w = weights(l)
                    for c in chunks:
                        wait_chunk(l - 1, c)
                    extended = l == 1 and me_ in (A_, B_) and chunks[0] >= N_LONG
                    if extended and not have_ext:
                        wait_bytes(wext, w_recv)
                        have_ext = True
                    a = jnp.concatenate([reduce_chunk(l - 1, c) for c in chunks], axis=0)
                    p = mlp(a.astype(bf16), w, extended)
                    for k, c in enumerate(chunks):
                        store_partial(l, c * R, p[k * R:(k + 1) * R])
                    run(l, script)

            def wait_sends(l):
                for copy in in_flight[l]:
                    copy.wait_send()

            for peer in HELLO[me_]:
                signal(barrier, peer)
            if me_ == D_:
                _SEM.semaphore_wait(barrier, 3)
                signal(d_ready, R_)

            load_x0.wait()
            load_w[0][0].wait()
            for l in (1, 2):
                load_w[l][0].start()
                load_w[l][1].start()
            for h in range(2):
                wib[0, h] = wiv[0, :, pl.ds(h * HH, HH)].astype(bf16)
            a = xv[pl.ds(0, R), :].astype(bf16)
            h0 = jnp.maximum(dot(a, wib[0, 0]), 0.0).astype(bf16)
            h1 = jnp.maximum(dot(a, wib[0, 1]), 0.0).astype(bf16)
            load_w[0][1].wait()
            w2 = wov[0, pl.ds(0, HH), :].astype(bf16)
            w3 = wov[0, pl.ds(HH, HH), :].astype(bf16)
            wob[0, pl.ds(0, HH), :] = w2
            wob[0, pl.ds(HH, HH), :] = w3
            store_partial(0, 0, dot(h0, w2) + dot(h1, w3))
            run(0, LAYER0[me_][0])
            load_x1.wait()
            store_partial(0, R, mlp(xv[pl.ds(R, B - R), :].astype(bf16), weights(0)))
            if me_ == R_:
                cast_weights(1)
            run(0, LAYER0[me_][1])
            if me_ != R_:
                cast_weights(1)

            layer(1, LAYER1[me_])
            cast_weights(2)
            wait_sends(0)
            layer(2, LAYER2[me_])
            wait_sends(1)
            order = [c for chunks, _ in LAYER2[me_] for c in chunks]
            for c in order:
                if c == order[-1]:
                    wait_sends(2)
                wait_chunk(2, c)
                out_ref[pl.ds(c * R, R), :] = reduce_chunk(2, c)

        for pos in (D_, A_, B_, R_):
            @pl.when(me == pos)
            def _():
                program(pos)

    known = {f.name for f in dataclasses.fields(pltpu.CompilerParams)}
    params = dict(collective_id=0, disable_bounds_checks=True, disable_semaphore_checks=True)

    return pl.pallas_call(
        body,
        out_shape=jax.ShapeDtypeStruct((B, D), f32),
        in_specs=[pl.BlockSpec(memory_space=pltpu.MemorySpace.HBM)] * 7,
        out_specs=pl.BlockSpec(memory_space=pltpu.MemorySpace.VMEM),
        scratch_shapes=[
            pltpu.VMEM((B, D), f32),
            pltpu.VMEM((3, D, H), f32),
            pltpu.VMEM((3, H, D), f32),
            pltpu.VMEM((3, 2, D, HH), bf16),
            pltpu.VMEM((3, H, D), bf16),
            pltpu.VMEM((2, D, HH), bf16),
            pltpu.VMEM((B, D), f32),
            pltpu.VMEM((3, B, D), bf16),
            pltpu.VMEM((B, D), bf16),
            pltpu.VMEM((3, 3 * B, D), bf16),
            pltpu.SemaphoreType.DMA((8,)),
            pltpu.SemaphoreType.DMA((3,)),
            pltpu.SemaphoreType.DMA((3, N_CHUNKS)),
            pltpu.SemaphoreType.DMA((N_CHUNKS,)),
            pltpu.SemaphoreType.DMA,
            pltpu.SemaphoreType.REGULAR,
        ],
        compiler_params=pltpu.CompilerParams(**{k: v for k, v in params.items() if k in known}),
    )(x, Win0, Wout0, Win1, Wout1, Win2, Wout2)
```
